```python
import numpy as np

kernel_name = "dist_sparse_attn_blocksparse_qseq_b2_sq256_skv256_hq4_dh64"

def setup_inputs():
    x = np.random.randn(2, 1024, 512).astype(np.float32)
    Wq = np.random.randn(512, 1024).astype(np.float32) * 0.02
    K_ext = np.random.randn(2, 256, 16, 64).astype(np.float32)
    V_ext = np.random.randn(2, 256, 16, 64).astype(np.float32)
    Wo = np.random.randn(1024, 512).astype(np.float32) * 0.02
    return {"x": x, "Wq": Wq, "K_ext": K_ext, "V_ext": V_ext, "Wo": Wo}

def reference(x, Wq, K_ext, V_ext, Wo):
    B, Sq, Skv, Hq, Dh = 2, 1024, 256, 16, 64
    Q = (x @ Wq).reshape(B, Sq, Hq, Dh)
    qb = (np.arange(Sq) // 64)[:, None]
    kb = (np.arange(Skv) // 64)[None, :]
    mask = (qb == kb) | (kb == 0) | ((qb + kb) % 3 == 0)
    scores = np.einsum('bihd,bjhd->bhij', Q, K_ext).astype(np.float32) * 0.125
    scores = np.where(mask[None, None, :, :], scores, -1e9)
    scores_max = scores.max(axis=-1, keepdims=True)
    w = np.exp(scores - scores_max)
    row_keep = mask.any(axis=1)
    w_sum = np.where(row_keep[None, None, :, None], w.sum(axis=-1, keepdims=True), 1.0)
    w = w / w_sum
    w = np.where(row_keep[None, None, :, None], w, 0.0)
    ctx = np.einsum('bhij,bjhd->bihd', w, V_ext).reshape(B, Sq, Hq * Dh)
    return ctx @ Wo
```

```python
import functools
import math

import jax
import jax.numpy as jnp
from jax import lax
from jax.experimental import pallas as pl
from jax.experimental.pallas import tpu as pltpu

N_DEV = 4
B, SQ, DM = 2, 256, 512
SKV, DH, BLK = 256, 64, 64
PAIR = 2 * DH
ROWS = B * SQ
OWN, LEFT, RIGHT, DIAG = range(4)
MESH = pl.DeviceIdType.MESH
LOG2E = math.log2(math.e)
BF16, F32 = jnp.bfloat16, jnp.float32


def make(scopes=False, sem_checks=True):
    import contextlib

    def scope(name):
        return jax.named_scope(name) if scopes else contextlib.nullcontext()

    def body(x_hbm, wq_hbm, kt_hbm, vt_hbm, wo_hbm, o_ref,
             wq_f32, wo_f32, x_f32, kt_f32, vt_f32,
             wq_buf, wo_buf, x_bf, ctx_buf, acc,
             load_sem, send_sem, recv_sem):
        me = lax.axis_index("i")
        right = lax.rem(me + 1, N_DEV)
        left = lax.rem(me + 3, N_DEV)
        diag = lax.rem(me + 2, N_DEV)
        owner = (me, left, right, diag)

        ld_wq = [pltpu.make_async_copy(wq_hbm.at[:, pl.ds(p * PAIR, PAIR)], wq_f32.at[p], load_sem.at[p])
                 for p in range(2)]
        ld_wo = [pltpu.make_async_copy(wo_hbm.at[pl.ds(p * PAIR, PAIR)], wo_f32.at[p], load_sem.at[2 + p])
                 for p in range(2)]
        ld_x = pltpu.make_async_copy(x_hbm, x_f32, load_sem.at[4])
        ld_k, ld_v = [], []
        for s in range(4):
            rows = pl.ds(pl.multiple_of(owner[s] * 2 * PAIR, 2 * PAIR), 2 * PAIR)
            ld_k.append(pltpu.make_async_copy(kt_hbm.at[:, rows], kt_f32.at[s], load_sem.at[5 + 2 * s]))
            ld_v.append(pltpu.make_async_copy(vt_hbm.at[:, rows], vt_f32.at[s], load_sem.at[6 + 2 * s]))
        for c in ld_wq:
            c.start()

        barrier = pltpu.get_barrier_semaphore()
        for nb in (left, right):
            pl.semaphore_signal(barrier, inc=1, device_id=(nb,), device_id_type=MESH)

        for c in ld_wo + [ld_x]:
            c.start()
        for s in range(4):
            ld_k[s].start()
            ld_v[s].start()

        n_msg = [0]

        def remote(src, dst, to):
            i = n_msg[0]
            n_msg[0] += 1
            return pltpu.make_async_remote_copy(src, dst, send_sem.at[i], recv_sem.at[i],
                                                device_id=(to,), device_id_type=MESH)

        wq_r = [remote(wq_buf.at[OWN, p], wq_buf.at[LEFT, p], right) for p in (0, 1)]
        wq_l = [remote(wq_buf.at[OWN, p], wq_buf.at[RIGHT, p], left) for p in (1, 0)]
        wo_r = [remote(wo_buf.at[OWN, p], wo_buf.at[LEFT, p], right) for p in (0, 1)]
        wo_l = [remote(wo_buf.at[OWN, p], wo_buf.at[RIGHT, p], left) for p in (1, 0)]
        fq_r = remote(wq_buf.at[LEFT, 0], wq_buf.at[DIAG, 0], right)
        fq_l = remote(wq_buf.at[RIGHT, 1], wq_buf.at[DIAG, 1], left)
        fo_r = [remote(wo_buf.at[LEFT, 0, n], wo_buf.at[DIAG, 0, n], right) for n in range(4)]
        fo_l = [remote(wo_buf.at[RIGHT, 1, n], wo_buf.at[DIAG, 1, n], left) for n in range(4)]

        with scope("cvt_wq"):
            for p in range(2):
                ld_wq[p].wait()
                wq_buf[OWN, p] = wq_f32[p].astype(BF16)
        with scope("barrier"):
            pl.semaphore_wait(barrier, 2)
        for a, b in zip(wq_r, wq_l):
            a.start()
            b.start()
        with scope("cvt_wo"):
            for p in range(2):
                ld_wo[p].wait()
                for n in range(4):
                    wo_buf[OWN, p, n] = wo_f32[p, :, n * 128:(n + 1) * 128].astype(BF16)
        wo_r[0].start()
        wo_l[0].start()

        with scope("cvt_x"):
            ld_x.wait()
            for b in range(B):
                x_bf[b * SQ:(b + 1) * SQ] = x_f32[b].astype(BF16)

        lo = lax.broadcasted_iota(jnp.int32, (1, PAIR), 1) < DH
        kb = lax.broadcasted_iota(jnp.int32, (1, SKV), 1) // BLK
        keep = []
        for j in range(SQ // BLK):
            qb = me * (SQ // BLK) + j
            keep.append((kb == qb) | (kb == 0) | (lax.rem(qb + kb, 3) == 0))

        def attend(s, p):
            q = jnp.dot(x_bf[...], wq_buf[s, p], preferred_element_type=F32) * (0.125 * LOG2E)
            for b in range(B):
                qb_ = q[b * SQ:(b + 1) * SQ]
                q2 = jnp.concatenate([jnp.where(lo, qb_, 0.0), jnp.where(lo, 0.0, qb_)], axis=0).astype(BF16)
                kt = kt_f32[s, b, p * PAIR:(p + 1) * PAIR].astype(BF16)
                vt = vt_f32[s, b, p * PAIR:(p + 1) * PAIR].astype(BF16)
                sc = jnp.dot(q2, kt, preferred_element_type=F32)
                sc = jnp.concatenate(
                    [jnp.where(keep[j % 4], sc[j * BLK:(j + 1) * BLK], -1e9 * LOG2E) for j in range(8)], axis=0)
                e = jnp.exp2(sc - jnp.max(sc, axis=1, keepdims=True))
                den = jnp.sum(e, axis=1, keepdims=True)
                pv = lax.dot_general(e.astype(BF16), vt, (((1,), (1,)), ((), ())), preferred_element_type=F32)
                pv = pv / den
                ctx_buf[s, p, b * SQ:(b + 1) * SQ] = jnp.where(lo, pv[:SQ], pv[SQ:]).astype(BF16)

        def project(items, n):
            lhs = jnp.concatenate([ctx_buf[s, p] for s, p in items], axis=1)
            rhs = jnp.concatenate([wo_buf[s, p, n] for s, p in items], axis=0)
            return jnp.dot(lhs, rhs, preferred_element_type=F32)

        with scope("att_own"):
            ld_k[OWN].wait()
            ld_v[OWN].wait()
            attend(OWN, 0)
            attend(OWN, 1)

        with scope("w_q1"):
            wq_r[0].wait_recv()
            wq_l[0].wait_recv()
        fq_r.start()
        fq_l.start()
        wo_r[1].start()
        wo_l[1].start()

        with scope("att_n0"):
            for s in (LEFT, RIGHT):
                ld_k[s].wait()
                ld_v[s].wait()
            attend(LEFT, 0)
            attend(RIGHT, 1)
        with scope("w_q2"):
            wq_r[1].wait_recv()
            wq_l[1].wait_recv()
        with scope("att_n1"):
            attend(LEFT, 1)
            attend(RIGHT, 0)

        with scope("w_o1"):
            wo_r[0].wait_recv()
            wo_l[0].wait_recv()
        for a, b in zip(fo_r, fo_l):
            a.start()
            b.start()
        with scope("proj1"):
            for n in range(4):
                acc[n] = project([(OWN, 0), (OWN, 1), (LEFT, 0), (RIGHT, 1)], n)

        with scope("w_qd"):
            fq_r.wait_recv()
            fq_l.wait_recv()
        with scope("att_d"):
            ld_k[DIAG].wait()
            ld_v[DIAG].wait()
            attend(DIAG, 0)
            attend(DIAG, 1)

        with scope("w_o2"):
            wo_r[1].wait_recv()
            wo_l[1].wait_recv()
        with scope("proj2"):
            for n in range(4):
                acc[n] += project([(LEFT, 1), (RIGHT, 0)], n)

        for c in wq_r + wq_l + wo_r + wo_l + [fq_r, fq_l]:
            c.wait_send()
        for n in range(4):
            with scope(f"w_d{n}"):
                if n == 3:
                    for c in fo_r[:3] + fo_l[:3]:
                        c.wait_send()
                fo_r[n].wait_recv()
                fo_l[n].wait_recv()
            with scope(f"fin{n}"):
                out = (acc[n] + project([(DIAG, 0), (DIAG, 1)], n)).astype(o_ref.dtype)
                for b in range(B):
                    o_ref[b, :, n * 128:(n + 1) * 128] = out[b * SQ:(b + 1) * SQ]
        fo_r[3].wait_send()
        fo_l[3].wait_send()
        assert n_msg[0] == 18

    def fn(x, Wq, K_ext, V_ext, Wo):
        kt = K_ext.transpose(0, 2, 3, 1).reshape(B, -1, SKV)
        vt = V_ext.transpose(0, 2, 3, 1).reshape(B, -1, SKV)
        hbm = pl.BlockSpec(memory_space=pltpu.HBM)
        return pl.pallas_call(
            body,
            out_shape=jax.ShapeDtypeStruct((B, SQ, DM), BF16),
            in_specs=[hbm] * 5,
            out_specs=pl.BlockSpec(memory_space=pltpu.VMEM),
            scratch_shapes=[
                pltpu.VMEM((2, DM, PAIR), F32),
                pltpu.VMEM((2, PAIR, DM), F32),
                pltpu.VMEM((B, SQ, DM), F32),
                pltpu.VMEM((4, B, 2 * PAIR, SKV), F32),
                pltpu.VMEM((4, B, 2 * PAIR, SKV), F32),
                pltpu.VMEM((4, 2, DM, PAIR), BF16),
                pltpu.VMEM((4, 2, 4, PAIR, 128), BF16),
                pltpu.VMEM((ROWS, DM), BF16),
                pltpu.VMEM((4, 2, ROWS, PAIR), BF16),
                pltpu.VMEM((4, ROWS, 128), F32),
                pltpu.SemaphoreType.DMA((13,)),
                pltpu.SemaphoreType.DMA((18,)),
                pltpu.SemaphoreType.DMA((18,)),
            ],
            compiler_params=pltpu.CompilerParams(
                collective_id=0, vmem_limit_bytes=48 << 20,
                disable_semaphore_checks=not sem_checks, disable_bounds_checks=not sem_checks),
        )(x, Wq, kt, vt, Wo)

    return fn


_kernel = make(scopes=False, sem_checks=False)


def pallas_dist_sparse_attn_blocksparse_qseq_b2_sq256_skv256_hq4_dh64_kernel(x, Wq, K_ext, V_ext, Wo):
    return _kernel(x, Wq, K_ext, V_ext, Wo)
```

```python
import contextlib
import math

import jax
import jax.numpy as jnp
from jax import lax
from jax.experimental import pallas as pl
from jax.experimental.pallas import tpu as pltpu

N_DEV = 4
B, SQ, DM = 2, 256, 512
SKV, DH, BLK = 256, 64, 64
PAIR = 2 * DH
ROWS = B * SQ
OWN, NY, NX, DIAG = range(4)
WQ, WO = range(2)
MESH = pl.DeviceIdType.MESH
LOG2E = math.log2(math.e)
BF16, F32, I32 = jnp.bfloat16, jnp.float32, jnp.int32
NT = (((1,), (1,)), ((), ()))


def i32(v):
    return v - (1 << 32) if v >= (1 << 31) else v


def words(v):
    return pltpu.bitcast(v.astype(BF16), I32)


def halves(w):
    return pltpu.bitcast(w, BF16)


shl = lax.shift_left
shr = lax.shift_right_logical
SPARE = 0x78007800
COUNT = 0x07FF0000


def pack_quad(w, offset, k, book):
    t = [w[8 * j:8 * j + 8] - offset for j in range(4)]
    h = [v & SPARE for v in t]
    top, total = book
    for j in range(4):
        key = jnp.where(h[j] != 0, h[j] | ((1 << 16) | (k + j)), 0)
        top = key if top is None else jnp.maximum(top, key)
        total = key if total is None else total + key
    d = t[3]
    z = [(t[0] ^ h[0]) | (shl(d, 11) & SPARE),
         (t[1] ^ h[1]) | (shl(d, 7) & SPARE),
         (t[2] ^ h[2]) | (shl(d, 3) & 0x38003800) | (shr(d, 1) & 0x40004000)]
    return jnp.concatenate(z, axis=0), (top, total)


def unpack_quad(z, k, table):
    c, c0, c1, k0, k1 = table
    z = [z[8 * j:8 * j + 8] for j in range(3)]
    h = [v & SPARE for v in z]
    t = [v ^ u for v, u in zip(z, h)]
    t.append(shr(h[0], 11) | shr(h[1], 7) | (shr(h[2], 3) & 0x07000700) | (shl(h[2], 1) & i32(0x80008000)))
    return jnp.concatenate(
        [t[j] + jnp.where(k0 == k + j, c0, jnp.where(k1 == k + j, c1, c)) for j in range(4)], axis=0)


def make(scopes=False, sem_checks=False, cuts=(0, 1, 3, 8), wo_pre=4, force_raw=False):
    def scope(name):
        return jax.named_scope(name) if scopes else contextlib.nullcontext()

    spans = list(zip(cuts, cuts[1:]))
    n_remote = 2 * len(spans) + 2 + 2 + 2 + 2 + 2 + 3 + 8 + 4

    def body(x_hbm, wq_hbm, kt_hbm, vt_hbm, wo_hbm, o_ref,
             wq_f32, wo_f32, x_f32, kt_f32, vt_f32,
             raw, packed, side, x_bf, ctx_buf, acc,
             load_sem, send_sem, recv_sem, ready_sem):
        me = lax.axis_index("i")
        ny = jnp.bitwise_xor(me, 1)
        nx = jnp.bitwise_xor(me, 3)
        owner = (me, ny, nx, jnp.bitwise_xor(me, 2))

        n_ld = [0]

        def local(src, dst):
            i = n_ld[0]
            n_ld[0] += 1
            return pltpu.make_async_copy(src, dst, load_sem.at[i])

        ld_wq = [local(wq_hbm.at[pl.ds(64 * a, 64 * (b - a))], wq_f32.at[pl.ds(64 * a, 64 * (b - a))])
                 for a, b in spans]
        ld_wo = [local(wo_hbm.at[pl.ds(p * PAIR, PAIR)], wo_f32.at[p]) for p in range(2)]
        ld_x = local(x_hbm, x_f32)
        order = [(OWN, 0), (OWN, 1), (NY, 0), (NX, 1), (NY, 1), (NX, 0), (DIAG, 0), (DIAG, 1)]
        ld_k, ld_v = {}, {}
        for s, p in order:
            rows = pl.ds(pl.multiple_of((owner[s] * 2 + p) * PAIR, PAIR), PAIR)
            ld_k[s, p] = local(kt_hbm.at[:, rows], kt_f32.at[s, p])
            ld_v[s, p] = local(vt_hbm.at[:, rows], vt_f32.at[s, p])
        ld_wq[0].start()

        barrier = pltpu.get_barrier_semaphore()

        def signal_both(sem):
            for nb in (ny, nx):
                pl.semaphore_signal(sem, inc=1, device_id=(nb,), device_id_type=MESH)

        pl.when(me != 2)(lambda: signal_both(barrier))

        for c in ld_wq[1:] + ld_wo + [ld_x]:
            c.start()
        for sp in order:
            ld_k[sp].start()
            ld_v[sp].start()

        @pl.when(me == 2)
        def _():
            pl.semaphore_wait(barrier, 2)
            signal_both(ready_sem)

        n_msg = [0]

        def remote(src, dst, to):
            i = n_msg[0]
            n_msg[0] += 1
            return pltpu.make_async_remote_copy(src, dst, send_sem.at[i], recv_sem.at[i],
                                                device_id=(to,), device_id_type=MESH)

        def quads(slot, p, m, a, b):
            return packed.at[slot, p, m, pl.ds(24 * a, 24 * (b - a))]

        def send(src, dst, to, p, m, a=0, b=8):
            return remote(quads(src, p, m, a, b), quads(dst, p, m, a, b), to)

        cut = 2 * wo_pre
        wq_y0 = [send(OWN, NY, ny, 0, WQ, a, b) for a, b in spans]
        wq_x0 = [send(OWN, NX, nx, 1, WQ, a, b) for a, b in spans]
        side_y = remote(side.at[OWN], side.at[NY], ny)
        side_x = remote(side.at[OWN], side.at[NX], nx)
        wq_y1, wq_x1 = send(OWN, NY, ny, 1, WQ), send(OWN, NX, nx, 0, WQ)
        wo_y0a = [send(OWN, NY, ny, 0, WO, 0, cut)] if cut > 0 else []
        wo_x0a = [send(OWN, NX, nx, 1, WO, 0, cut)] if cut > 0 else []
        wo_y0b = [send(OWN, NY, ny, 0, WO, cut, 8)] if cut < 8 else []
        wo_x0b = [send(OWN, NX, nx, 1, WO, cut, 8)] if cut < 8 else []
        wo_y1, wo_x1 = send(OWN, NY, ny, 1, WO), send(OWN, NX, nx, 0, WO)
        fs_x = remote(side.at[NY], side.at[DIAG], nx)
        fq_x, fq_y = send(NY, DIAG, nx, 0, WQ), send(NX, DIAG, ny, 1, WQ)
        fo_x = [send(NY, DIAG, nx, 0, WO, 2 * n, 2 * n + 2) for n in range(4)]
        fo_y = [send(NX, DIAG, ny, 1, WO, 2 * n, 2 * n + 2) for n in range(4)]
        raw_y = remote(raw.at[OWN], raw.at[NY], ny)
        raw_x = remote(raw.at[OWN], raw.at[NX], nx)
        fraw_x = remote(raw.at[NY, 0], raw.at[DIAG, 0], nx)
        fraw_y = remote(raw.at[NX, 1], raw.at[DIAG, 1], ny)
        assert n_msg[0] <= n_remote

        book = (None, None)

        def pack(v, p, m, q, book):
            w = words(v)
            raw[OWN, p, m, 32 * q:32 * q + 32] = w
            z, book = pack_quad(w, offset, ((2 * p + m) * 8 + q) * 4, book)
            packed[OWN, p, m, 24 * q:24 * q + 24] = z
            return book

        for i, (a, b) in enumerate(spans):
            with scope(f"cvt_wq{i}"):
                ld_wq[i].wait()
                if i == 0:
                    peak = jnp.max(jnp.abs(wq_f32[0:64 * b]), axis=0, keepdims=True)
                    peak = jnp.broadcast_to(jnp.max(peak, axis=1, keepdims=True), (8, 128))
                    base = (shr(pltpu.bitcast(peak * 1.15, I32), 23) - 15) & 0xFF
                    offset = shl(base, 7) | shl(base, 23)
                for q in range(a, b):
                    for p in range(2):
                        book = pack(wq_f32[64 * q:64 * q + 64, p * PAIR:(p + 1) * PAIR], p, WQ, q, book)
            if i == 0:
                with scope("barrier"):
                    pl.when(me == 0)(lambda: pl.semaphore_wait(barrier, 2))
                    pl.when(lax.rem(me, 2) == 1)(lambda: pl.semaphore_wait(barrier, 1))
            pl.when(me != 3)(wq_y0[i].start)
            pl.when(me != 1)(wq_x0[i].start)

        with scope("ready"):
            @pl.when(me == 3)
            def _():
                pl.semaphore_wait(ready_sem, 1)
                for c in wq_y0:
                    c.start()

            @pl.when(me == 1)
            def _():
                pl.semaphore_wait(ready_sem, 1)
                for c in wq_x0:
                    c.start()

        with scope("cvt_wo"):
            for p in range(2):
                ld_wo[p].wait()
                for q in range(8):
                    n, r = q // 2, q % 2
                    book = pack(wo_f32[p, 64 * r:64 * r + 64, n * 128:(n + 1) * 128], p, WO, q, book)
            top, total = book
            second = total - top
            spill = jnp.where((total & COUNT) > (2 << 16), 1, 0)
            if force_raw:
                spill = spill | 1
            spill = jnp.max(jnp.max(spill, axis=0, keepdims=True), axis=1, keepdims=True)
            sub = lax.broadcasted_iota(I32, (8, 128), 0)
            side[OWN] = ((top & 0x7800787F) | shr(second & SPARE, 4) | shl(second & 0x7F, 16)
                         | shl(shr(base, sub) & 1, 15) | shl(jnp.broadcast_to(spill, (8, 128)), 31))
        for c in [side_y, side_x, wq_y1, wq_x1] + wo_y0a + wo_x0a:
            c.start()

        def read_side(s):
            v = side[s]
            base = jnp.sum(shl(shr(v, 15) & 1, sub), axis=0, keepdims=True)
            c = jnp.broadcast_to(shl(base, 7) | shl(base, 23), (8, 128))
            table = (c, c + (v & SPARE), c + (shl(v, 4) & SPARE), v & 0x7F, shr(v, 16) & 0x7F)
            return table, v < 0, v[0, 0] < 0

        is_raw = {OWN: spill[0, 0] > 0}

        @pl.when(is_raw[OWN])
        def _():
            raw_y.start()
            raw_x.start()

        with scope("cvt_x"):
            ld_x.wait()
            for b in range(B):
                x_bf[b] = words(x_f32[b] * (0.125 * LOG2E))

        tables, raw_mask = {}, {}

        def weights(s, p, m, a=0, b=8):
            if s == OWN:
                return halves(raw[s, p, m, 32 * a:32 * b])
            w = [jnp.where(raw_mask[s], raw[s, p, m, 32 * q + 8 * j:32 * q + 8 * j + 8], v[8 * j:8 * j + 8])
                 for q in range(a, b)
                 for v in [unpack_quad(packed[s, p, m, 24 * q:24 * q + 24], ((2 * p + m) * 8 + q) * 4, tables[s])]
                 for j in range(4)]
            return halves(jnp.concatenate(w, axis=0))

        lo = lax.broadcasted_iota(I32, (1, PAIR), 1) < DH
        kb = lax.broadcasted_iota(I32, (1, SKV), 1) // BLK
        keep = {}
        for j in (1, 2):
            qb = me * (SQ // BLK) + j
            keep[j] = (kb == qb) | (kb == 0) | (lax.rem(qb + kb, 3) == 0)
        kb2 = 3 - lax.rem(me, 3)
        take0 = lo | (kb2 == 1)
        take_rolled = jnp.broadcast_to(kb2 == 2, (1, PAIR))

        def key_tiles(ref, s, b, p):
            t0 = ref[s, p, b, :, 0:128]
            t1 = ref[s, p, b, :, 128:256]
            sel = jnp.where(take0, t0, jnp.where(take_rolled, pltpu.roll(t1, DH, 1), t1))
            return sel.astype(BF16), jnp.concatenate([t0, t1], axis=1).astype(BF16)

        def queries(s, p):
            xs = jnp.concatenate([halves(x_bf[b]) for b in range(B)], axis=0)
            return jnp.dot(xs, weights(s, p, WQ), preferred_element_type=F32)

        def scores(q, s, p):
            out = []
            for b in range(B):
                qj = [q[(b * 4 + j) * BLK:(b * 4 + j + 1) * BLK] for j in range(4)]

                def two_heads(js):
                    qq = jnp.concatenate([qj[j] for j in js], axis=0)
                    return jnp.concatenate([jnp.where(lo, qq, 0.0), jnp.where(lo, 0.0, qq)], axis=0).astype(BF16)

                k_sel, k_all = key_tiles(kt_f32, s, b, p)
                out.append((jnp.dot(two_heads((0, 3)), k_sel, preferred_element_type=F32),
                            jnp.dot(two_heads((1, 2)), k_all, preferred_element_type=F32)))
            return out

        def softmax_pv(sc, vt):
            e = jnp.exp2(sc - jnp.max(sc, axis=1, keepdims=True))
            den = jnp.sum(e, axis=1, keepdims=True)
            pv = lax.dot_general(e.astype(BF16), vt, NT, preferred_element_type=F32)
            h = pv.shape[0] // 2
            num = jnp.where(lo, pv[:h], pv[h:])
            den = jnp.where(lo, den[:h], den[h:])
            r = pl.reciprocal(den, approx=True)
            r = r * (2.0 - den * r)
            return words(num * r)

        def context(sc, s, p):
            hb = BLK // 2
            for b in range(B):
                s03, s12 = sc[b]
                v_sel, v_all = key_tiles(vt_f32, s, b, p)
                c03 = softmax_pv(s03, v_sel)
                s12 = jnp.concatenate(
                    [jnp.where(keep[1 + j % 2], s12[j * BLK:(j + 1) * BLK], -1e9 * LOG2E) for j in range(4)], axis=0)
                c12 = softmax_pv(s12, v_all)
                ctx_buf[s, p, b, 0:hb] = c03[:hb]
                ctx_buf[s, p, b, hb:3 * hb] = c12
                ctx_buf[s, p, b, 3 * hb:4 * hb] = c03[hb:]

        def project(items, n, bs=(0, 1), rhs=None):
            lhs = jnp.concatenate(
                [jnp.concatenate([halves(ctx_buf[s, p, b]) for b in bs], axis=0) for s, p in items], axis=1)
            if rhs is None:
                rhs = jnp.concatenate([weights(s, p, WO, 2 * n, 2 * n + 2) for s, p in items], axis=0)
            return jnp.dot(lhs, rhs, preferred_element_type=F32)

        def landed(ks, vs):
            for sp in ks:
                ld_k[sp].wait()
            for sp in vs:
                ld_v[sp].wait()

        def step(sc, cur, nxt):
            q = queries(*nxt)
            context(sc, *cur)
            return scores(q, *nxt)

        with scope("q_own"):
            q = queries(*order[0])
        with scope("att_own"):
            landed(order[0:1], [])
            sc = scores(q, *order[0])
            landed(order[1:2], order[0:1])
            sc = step(sc, order[0], order[1])

        with scope("w_q1"):
            for c in wq_y0 + wq_x0 + [side_y, side_x]:
                c.wait_recv()
        for c in [fs_x, fq_x, fq_y] + wo_y0b + wo_x0b + [wo_y1, wo_x1]:
            c.start()
        for s in (NY, NX):
            tables[s], raw_mask[s], is_raw[s] = read_side(s)

        @pl.when(is_raw[NY])
        def _():
            raw_y.wait_recv()
            fraw_x.start()

        @pl.when(is_raw[NX])
        def _():
            raw_x.wait_recv()
            fraw_y.start()

        with scope("att_n0"):
            landed(order[2:3], order[1:2])
            sc = step(sc, order[1], order[2])
            landed(order[3:4], order[2:3])
            sc = step(sc, order[2], order[3])
        with scope("w_q2"):
            wq_y1.wait_recv()
            wq_x1.wait_recv()
            landed(order[4:6], order[3:5])
        with scope("att_n1"):
            sc = step(sc, order[3], order[4])
            sc = step(sc, order[4], order[5])

        with scope("w_o1"):
            landed(order[6:8], order[5:8])
            for c in wo_y0a + wo_x0a + wo_y0b + wo_x0b:
                c.wait_recv()
        for a, b in zip(fo_x, fo_y):
            a.start()
            b.start()
        with scope("proj1"):
            for n in range(4):
                acc[n] = project([(OWN, 0), (OWN, 1), (NY, 0), (NX, 1)], n)
                if n == 0:
                    context(sc, NX, 0)

        with scope("w_qd"):
            for c in (fs_x, fq_x, fq_y):
                c.wait_recv()
        tables[DIAG], raw_mask[DIAG], is_raw[DIAG] = read_side(DIAG)

        @pl.when(is_raw[DIAG])
        def _():
            fraw_x.wait_recv()
            fraw_y.wait_recv()

        with scope("att_d"):
            sc = scores(queries(DIAG, 0), DIAG, 0)
            sc = step(sc, order[6], order[7])

        with scope("w_o2"):
            wo_y1.wait_recv()
            wo_x1.wait_recv()
        with scope("proj2"):
            for n in range(4):
                acc[n] += project([(NY, 1), (NX, 0)], n)
                if n == 1:
                    context(sc, DIAG, 1)

        for c in (wq_y0 + wq_x0 + [side_y, side_x, wq_y1, wq_x1] + wo_y0a + wo_x0a + wo_y0b + wo_x0b
                  + [wo_y1, wo_x1, fs_x, fq_x, fq_y]):
            c.wait_send()

        @pl.when(is_raw[OWN])
        def _():
            raw_y.wait_send()
            raw_x.wait_send()

        pl.when(is_raw[NY])(fraw_x.wait_send)
        pl.when(is_raw[NX])(fraw_y.wait_send)

        for n in range(4):
            with scope(f"w_d{n}"):
                if n == 3:
                    for c in fo_x[:3] + fo_y[:3]:
                        c.wait_send()
                fo_x[n].wait_recv()
                fo_y[n].wait_recv()
            with scope(f"fin{n}"):
                rhs = jnp.concatenate([weights(DIAG, p, WO, 2 * n, 2 * n + 2) for p in range(2)], axis=0)
                for b in range(B):
                    out = acc[n, b * SQ:(b + 1) * SQ] + project([(DIAG, 0), (DIAG, 1)], n, (b,), rhs)
                    o_ref[b, :, n * 128:(n + 1) * 128] = out.astype(o_ref.dtype)
        fo_x[3].wait_send()
        fo_y[3].wait_send()

    def fn(x, Wq, K_ext, V_ext, Wo):
        kt = K_ext.transpose(0, 2, 3, 1).reshape(B, -1, SKV)
        vt = V_ext.transpose(0, 2, 3, 1).reshape(B, -1, SKV)
        hbm = pl.BlockSpec(memory_space=pltpu.HBM)
        return pl.pallas_call(
            body,
            out_shape=jax.ShapeDtypeStruct((B, SQ, DM), BF16),
            in_specs=[hbm] * 5,
            out_specs=pl.BlockSpec(memory_space=pltpu.VMEM),
            scratch_shapes=[
                pltpu.VMEM((DM, 2 * PAIR), F32),
                pltpu.VMEM((2, PAIR, DM), F32),
                pltpu.VMEM((B, SQ, DM), F32),
                pltpu.VMEM((4, 2, B, PAIR, SKV), F32),
                pltpu.VMEM((4, 2, B, PAIR, SKV), F32),
                pltpu.VMEM((4, 2, 2, 256, 128), I32),
                pltpu.VMEM((4, 2, 2, 192, 128), I32),
                pltpu.VMEM((4, 8, 128), I32),
                pltpu.VMEM((B, SQ // 2, DM), I32),
                pltpu.VMEM((4, 2, B, SQ // 2, PAIR), I32),
                pltpu.VMEM((4, ROWS, 128), F32),
                pltpu.SemaphoreType.DMA((len(spans) + 19,)),
                pltpu.SemaphoreType.DMA((n_remote,)),
                pltpu.SemaphoreType.DMA((n_remote,)),
                pltpu.SemaphoreType.REGULAR,
            ],
            compiler_params=pltpu.CompilerParams(
                collective_id=0, vmem_limit_bytes=48 << 20,
                disable_semaphore_checks=not sem_checks, disable_bounds_checks=not sem_checks),
        )(x, Wq, kt, vt, Wo)

    return fn


_kernel = make()


def pallas_dist_sparse_attn_blocksparse_qseq_b2_sq256_skv256_hq4_dh64_kernel(x, Wq, K_ext, V_ext, Wo):
    return _kernel(x, Wq, K_ext, V_ext, Wo)
```

```python
import math

import jax
import jax.numpy as jnp
from jax import lax
from jax.experimental import pallas as pl
from jax.experimental.pallas import tpu as pltpu

B, SQ, DM = 2, 256, 512
SKV, DH, BLK = 256, 64, 64
PAIR = 2 * DH
Q_SCALE = 0.125 * math.log2(math.e)
MASKED = -1e9 * math.log2(math.e)

OWN, NY, NX, DIAG = range(4)
WQ, WO = range(2)
ORDER = ((OWN, 0), (OWN, 1), (NY, 0), (NX, 1), (NY, 1), (NX, 0), (DIAG, 0), (DIAG, 1))
HEAD = ((0, 1), (1, 3), (3, 8))
HEAD_LOADS = ((0, 0), (0, 1), (1, 0), (0, 2), (1, 1), (1, 2))

BF16, F32, I32 = jnp.bfloat16, jnp.float32, jnp.int32
MESH = pl.DeviceIdType.MESH
shl, shr = lax.shift_left, lax.shift_right_logical

SPARE = 0x78007800
SIGNS = 0x80008000 - (1 << 32)
INDEX = 0x7F
ONE, COUNT = 0x00010000, 0x07FF0000


def _words(v):
    return pltpu.bitcast(v.astype(BF16), I32)


def _halves(w):
    return pltpu.bitcast(w, BF16)


def _window(sample):
    peak = jnp.max(jnp.max(jnp.abs(sample), axis=1, keepdims=True), axis=0, keepdims=True)
    peak = jnp.broadcast_to(peak * 1.25, (8, 128))
    return (shr(pltpu.bitcast(peak, I32), 23) - 15) & 0xFF


def _offset(window):
    return shl(window, 7) | shl(window, 23)


def _pack_quad(w, offset, k, book):
    t = [w[8 * j:8 * j + 8] - offset for j in range(4)]
    h = [v & SPARE for v in t]
    for j in range(4):
        key = jnp.where(h[j] != 0, h[j] | (ONE + k + j), 0)
        book = (key, key) if book is None else (jnp.maximum(book[0], key), book[1] + key)
    z = [(t[0] ^ h[0]) | (shl(t[3], 11) & SPARE),
         (t[1] ^ h[1]) | (shl(t[3], 7) & SPARE),
         (t[2] ^ h[2]) | (shl(t[3], 3) & 0x38003800) | (shr(t[3], 1) & 0x40004000)]
    return jnp.concatenate(z, axis=0), book


def _unpack_quad(z, offsets, k0, k1, k):
    c, c0, c1 = offsets
    z = [z[8 * j:8 * j + 8] for j in range(3)]
    h = [v & SPARE for v in z]
    t = [v ^ u for v, u in zip(z, h)]
    t.append(shr(h[0], 11) | shr(h[1], 7) | (shr(h[2], 3) & 0x07000700) | (shl(h[2], 1) & SIGNS))
    return [t[j] + jnp.where(k0 == k + j, c0, jnp.where(k1 == k + j, c1, c)) for j in range(4)]


def _side_table(book, windows):
    first, total = book
    second = total - first
    full = jnp.where((total & COUNT) > 2 * ONE, 1, 0)
    full = jnp.max(jnp.max(full, axis=0, keepdims=True), axis=1, keepdims=True)
    first = jnp.where(jnp.broadcast_to(full, (8, 128)) > 0, 1, first & (SPARE | INDEX))
    row = lax.broadcasted_iota(I32, (8, 128), 0)
    table = (first | shr(second & SPARE, 4) | shl(second & INDEX, 16)
             | shl(shr(windows[WQ], row) & 1, 15) | shl(shr(windows[WO], row), 31))
    return table, full[0, 0] > 0


def _read_side_table(v):
    row = lax.broadcasted_iota(I32, (8, 128), 0)
    offsets = []
    for bit in (15, 31):
        window = jnp.sum(shl(shr(v, bit) & 1, row), axis=0, keepdims=True)
        c = jnp.broadcast_to(_offset(window), (8, 128))
        offsets.append((c, c + (v & SPARE), c + (shl(v, 4) & SPARE)))
    entry = v & (SPARE | INDEX)
    return (offsets, v & INDEX, shr(v, 16) & INDEX, entry == 1), entry[0, 0] == 1


def _body(x_hbm, wq_hbm, kt_hbm, vt_hbm, wo_hbm, o_ref,
          peek, wq_f32, wo_f32, x_f32, kt_f32, vt_f32,
          plain, packed, side, x_bf, ctx_buf, acc,
          load_sem, send_sem, recv_sem, ready_sem):
    loads = []

    def load(src, dst):
        loads.append(pltpu.make_async_copy(src, dst, load_sem.at[len(loads)]))
        return loads[-1]

    ld_peek = load(wq_hbm.at[pl.ds(0, 8)], peek)
    ld_peek.start()

    me = lax.axis_index("i")
    ny, nx = me ^ 1, me ^ 3
    owner = (me, ny, nx, me ^ 2)
    odd = (me & 1) == 1
    link = (jnp.where(me == 3, 1, 0), jnp.where(me == 3, 0, 1))

    ld_wq = {}
    for i, j in HEAD_LOADS:
        rows = pl.ds(64 * HEAD[j][0], 64 * (HEAD[j][1] - HEAD[j][0]))
        cols = pl.ds(pl.multiple_of(link[i] * PAIR, PAIR), PAIR)
        ld_wq[i, j] = load(wq_hbm.at[rows, cols], wq_f32.at[i, rows])
    ld_wo = [load(wo_hbm.at[pl.ds(p * PAIR, PAIR)], wo_f32.at[p]) for p in range(2)]
    ld_x = load(x_hbm, x_f32)
    ld_k, ld_v = {}, {}
    for s, p in ORDER:
        rows = pl.ds(pl.multiple_of((owner[s] * 2 + p) * PAIR, PAIR), PAIR)
        ld_k[s, p] = load(kt_hbm.at[:, rows], kt_f32.at[s, p])
        ld_v[s, p] = load(vt_hbm.at[:, rows], vt_f32.at[s, p])
    loads[1].start()

    barrier = pltpu.get_barrier_semaphore()

    def signal_neighbours(sem):
        for to in (ny, nx):
            pl.semaphore_signal(sem, inc=1, device_id=(to,), device_id_type=MESH)

    pl.when(me != 2)(lambda: signal_neighbours(barrier))

    @pl.when(me == 2)
    def _():
        pl.semaphore_wait(barrier, 2)
        signal_neighbours(ready_sem)

    for c in loads[2:]:
        c.start()

    messages = []

    def message(src, dst, to):
        i = len(messages)
        messages.append(pltpu.make_async_remote_copy(
            src, dst, send_sem.at[i], recv_sem.at[i], device_id=(to,), device_id_type=MESH))
        return messages[-1]

    def quads(slot, p, m, a, b):
        return packed.at[slot, p, m, pl.ds(24 * a, 24 * (b - a))]

    def send(src, dst, to, p, m, a=0, b=8):
        return message(quads(src, p, m, a, b), quads(dst, p, m, a, b), to)

    wq_y0 = [send(OWN, NY, ny, 0, WQ, a, b) for a, b in HEAD]
    wq_x0 = [send(OWN, NX, nx, 1, WQ, a, b) for a, b in HEAD]
    side_y, side_x = message(side.at[OWN], side.at[NY], ny), message(side.at[OWN], side.at[NX], nx)
    wq_y1, wq_x1 = send(OWN, NY, ny, 1, WQ), send(OWN, NX, nx, 0, WQ)
    wo_y0, wo_x0 = send(OWN, NY, ny, 0, WO), send(OWN, NX, nx, 1, WO)
    relay_q = [message(side.at[NY, pl.ds(0, 4)], side.at[DIAG, pl.ds(0, 4)], nx),
               message(side.at[NX, pl.ds(4, 4)], side.at[DIAG, pl.ds(4, 4)], ny),
               send(NY, DIAG, nx, 0, WQ), send(NX, DIAG, ny, 1, WQ)]
    wo_y1, wo_x1 = send(OWN, NY, ny, 1, WO), send(OWN, NX, nx, 0, WO)
    relay_x = [send(NY, DIAG, nx, 0, WO, a, b) for a, b in ((0, 2), (2, 4), (4, 6), (6, 7), (7, 8))]
    relay_y = [send(NX, DIAG, ny, 1, WO, a, b) for a, b in ((0, 2), (2, 4), (4, 6), (7, 8), (6, 7))]
    plain_y, plain_x = message(plain.at[OWN], plain.at[NY], ny), message(plain.at[OWN], plain.at[NX], nx)
    relay_plain_x = message(plain.at[NY, 0], plain.at[DIAG, 0], nx)
    relay_plain_y = message(plain.at[NX, 1], plain.at[DIAG, 1], ny)

    def head(i, j):
        p = link[i]
        return pltpu.make_async_remote_copy(
            quads(OWN, p, WQ, *HEAD[j]), quads(NY + p, p, WQ, *HEAD[j]),
            send_sem.at[p * len(HEAD) + j], recv_sem.at[p * len(HEAD) + j],
            device_id=(jnp.where(p == 0, ny, nx),), device_id_type=MESH)

    def pack(v, offset, p, m, q, book):
        w = _words(v)
        plain[OWN, p, m, 32 * q:32 * q + 32] = w
        z, book = _pack_quad(w, offset, 64 * p + 32 * m + 4 * q, book)
        packed[OWN, p, m, 24 * q:24 * q + 24] = z
        return book

    pl.when(odd)(lambda: pl.semaphore_wait(barrier, 1))
    ld_peek.wait()
    window_q = _window(peek[...])
    offset, book = _offset(window_q), None
    for n, (i, j) in enumerate(HEAD_LOADS):
        ld_wq[i, j].wait()
        for q in range(*HEAD[j]):
            book = pack(wq_f32[i, 64 * q:64 * q + 64], offset, link[i], WQ, q, book)
        if n == 0:
            pl.when(me == 0)(lambda: pl.semaphore_wait(barrier, 2))
        if i == 0:
            head(i, j).start()
        else:
            pl.when(jnp.logical_not(odd))(head(i, j).start)

    @pl.when(odd)
    def _():
        pl.semaphore_wait(ready_sem, 1)
        for j in range(len(HEAD)):
            head(1, j).start()

    for p in range(2):
        ld_wo[p].wait()
        if p == 0:
            window_o = _window(wo_f32[0, 0:16])
            offset = _offset(window_o)
        for q in range(8):
            n, r = divmod(q, 2)
            book = pack(wo_f32[p, 64 * r:64 * r + 64, 128 * n:128 * n + 128], offset, p, WO, q, book)
    is_plain = {}
    side[OWN], is_plain[OWN] = _side_table(book, (window_q, window_o))
    for c in (side_y, side_x, wq_y1, wq_x1, wo_y0, wo_x0):
        c.start()

    @pl.when(is_plain[OWN])
    def _():
        plain_y.start()
        plain_x.start()

    ld_x.wait()
    for b in range(B):
        x_bf[b] = _words(x_f32[b] * Q_SCALE)

    tables = {}

    def weights(s, p, m, a=0, b=8):
        if s == OWN:
            return _halves(plain[s, p, m, 32 * a:32 * b])
        offsets, k0, k1, use_plain = tables[s]
        w = []
        for q in range(a, b):
            v = _unpack_quad(packed[s, p, m, 24 * q:24 * q + 24], offsets[m], k0, k1, 64 * p + 32 * m + 4 * q)
            w += [jnp.where(use_plain, plain[s, p, m, 32 * q + 8 * j:32 * q + 8 * j + 8], v[j]) for j in range(4)]
        return _halves(jnp.concatenate(w, axis=0))

    lo = lax.broadcasted_iota(I32, (1, PAIR), 1) < DH
    kb = lax.broadcasted_iota(I32, (1, SKV), 1) // BLK
    keep = [(kb == qb) | (kb == 0) | (lax.rem(qb + kb, 3) == 0) for qb in (4 * me + 1, 4 * me + 2)]
    kb2 = 3 - lax.rem(me, 3)
    take_first = lo | (kb2 == 1)
    take_rolled = jnp.broadcast_to(kb2 == 2, (1, PAIR))

    def key_tiles(ref, s, p, b):
        t0, t1 = ref[s, p, b, :, 0:128], ref[s, p, b, :, 128:256]
        two = jnp.where(take_first, t0, jnp.where(take_rolled, pltpu.roll(t1, BLK, 1), t1))
        return two.astype(BF16), jnp.concatenate([t0, t1], axis=1).astype(BF16)

    def queries(s, p):
        x = jnp.concatenate([_halves(x_bf[b]) for b in range(B)], axis=0)
        return jnp.dot(x, weights(s, p, WQ), preferred_element_type=F32)

    def scores(q, s, p):
        out = []
        for b in range(B):
            parts = []
            for blocks, kt in zip(((0, 3), (1, 2)), key_tiles(kt_f32, s, p, b)):
                v = jnp.concatenate([q[b * SQ + j * BLK:b * SQ + (j + 1) * BLK] for j in blocks], axis=0)
                v = jnp.concatenate([jnp.where(lo, v, 0.0), jnp.where(lo, 0.0, v)], axis=0)
                parts.append(jnp.dot(v.astype(BF16), kt, preferred_element_type=F32))
            out.append(parts)
        return out

    def softmax_pv(sc, vt):
        e = jnp.exp2(sc - jnp.max(sc, axis=1, keepdims=True))
        den = jnp.sum(e, axis=1, keepdims=True)
        num = lax.dot_general(e.astype(BF16), vt, (((1,), (1,)), ((), ())), preferred_element_type=F32)
        h = num.shape[0] // 2
        num, den = jnp.where(lo, num[:h], num[h:]), jnp.where(lo, den[:h], den[h:])
        r = pl.reciprocal(den, approx=True)
        r = r * (2.0 - den * r)
        return _words(num * r)

    def context(sc, s, p):
        h = BLK // 2
        for b in range(B):
            v_two, v_all = key_tiles(vt_f32, s, p, b)
            c03 = softmax_pv(sc[b][0], v_two)
            c12 = softmax_pv(jnp.concatenate(
                [jnp.where(keep[j % 2], sc[b][1][j * BLK:(j + 1) * BLK], MASKED) for j in range(4)], axis=0), v_all)
            ctx_buf[s, p, b, 0:h] = c03[:h]
            ctx_buf[s, p, b, h:3 * h] = c12
            ctx_buf[s, p, b, 3 * h:4 * h] = c03[h:]

    def project(items, batches, w):
        ctx = jnp.concatenate(
            [jnp.concatenate([_halves(ctx_buf[s, p, b]) for b in batches], axis=0) for s, p in items], axis=1)
        return jnp.dot(ctx, w, preferred_element_type=F32)

    def wo_block(items, n):
        return jnp.concatenate([weights(s, p, WO, 2 * n, 2 * n + 2) for s, p in items], axis=0)

    def wait_kv(keys, values):
        for sp in keys:
            ld_k[sp].wait()
        for sp in values:
            ld_v[sp].wait()

    def step(sc, i):
        q = queries(*ORDER[i + 1])
        context(sc, *ORDER[i])
        return scores(q, *ORDER[i + 1])

    q = queries(*ORDER[0])
    wait_kv(ORDER[0:1], ())
    sc = scores(q, *ORDER[0])
    wait_kv(ORDER[1:2], ORDER[0:1])
    sc = step(sc, 0)

    for c in wq_y0 + wq_x0 + [side_y, side_x]:
        c.wait_recv()
    for c in relay_q + [wo_y1, wo_x1]:
        c.start()
    for s in (NY, NX):
        tables[s], is_plain[s] = _read_side_table(side[s])

    @pl.when(is_plain[NY])
    def _():
        plain_y.wait_recv()
        relay_plain_x.start()

    @pl.when(is_plain[NX])
    def _():
        plain_x.wait_recv()
        relay_plain_y.start()

    wait_kv(ORDER[2:3], ORDER[1:2])
    sc = step(sc, 1)
    wait_kv(ORDER[3:4], ORDER[2:3])
    sc = step(sc, 2)

    wq_y1.wait_recv()
    wq_x1.wait_recv()
    wait_kv(ORDER[4:6], ORDER[3:5])
    sc = step(sc, 3)
    sc = step(sc, 4)

    wait_kv(ORDER[6:8], ORDER[5:8])
    wo_y0.wait_recv()
    wo_x0.wait_recv()
    for cx, cy in zip(relay_x, relay_y):
        cx.start()
        cy.start()
    for n in range(4):
        acc[n] = project(ORDER[0:4], range(B), wo_block(ORDER[0:4], n))
        if n == 0:
            context(sc, *ORDER[5])

    for c in relay_q:
        c.wait_recv()
    tables[DIAG], is_plain[DIAG] = _read_side_table(side[DIAG])

    @pl.when(is_plain[DIAG])
    def _():
        relay_plain_x.wait_recv()
        relay_plain_y.wait_recv()

    sc = scores(queries(*ORDER[6]), *ORDER[6])
    sc = step(sc, 6)
    context(sc, *ORDER[7])

    wo_y1.wait_recv()
    wo_x1.wait_recv()
    for n in range(4):
        acc[n] += project(ORDER[4:6], range(B), wo_block(ORDER[4:6], n))

    for c in wq_y0 + wq_x0 + [side_y, side_x, wq_y1, wq_x1, wo_y0, wo_x0, wo_y1, wo_x1] + relay_q:
        c.wait_send()

    @pl.when(is_plain[OWN])
    def _():
        plain_y.wait_send()
        plain_x.wait_send()

    pl.when(is_plain[NY])(relay_plain_x.wait_send)
    pl.when(is_plain[NX])(relay_plain_y.wait_send)

    for n in range(3):
        relay_x[n].wait_recv()
        relay_y[n].wait_recv()
        w = wo_block(ORDER[6:8], n)
        for b in range(B):
            out = acc[n, b * SQ:(b + 1) * SQ] + project(ORDER[6:8], (b,), w)
            o_ref[b, :, 128 * n:128 * n + 128] = out.astype(o_ref.dtype)

    for i in range(2):
        if i == 1:
            for c in relay_x[:4] + relay_y[:4]:
                c.wait_send()
        relay_x[3 + i].wait_recv()
        relay_y[3 + i].wait_recv()
        w = jnp.concatenate([weights(DIAG, i, WO, 6, 7), weights(DIAG, 1 - i, WO, 7, 8)], axis=0)
        for b in range(B):
            for r in range(2):
                h = slice(64 * r, 64 * r + 64)
                ctx = _halves(jnp.where(lo, ctx_buf[DIAG, i, b, h], ctx_buf[DIAG, 1 - i, b, h]))
                rows = slice(b * SQ + 128 * r, b * SQ + 128 * r + 128)
                out = acc[3, rows] + jnp.dot(ctx, w, preferred_element_type=F32)
                if i == 0:
                    acc[3, rows] = out
                else:
                    o_ref[b, 128 * r:128 * r + 128, 384:512] = out.astype(o_ref.dtype)
    relay_x[4].wait_send()
    relay_y[4].wait_send()


def pallas_dist_sparse_attn_blocksparse_qseq_b2_sq256_skv256_hq4_dh64_kernel(
    x: jax.Array,
    Wq: jax.Array,
    K_ext: jax.Array,
    V_ext: jax.Array,
    Wo: jax.Array,
):
    kt = K_ext.transpose(0, 2, 3, 1).reshape(B, -1, SKV)
    vt = V_ext.transpose(0, 2, 3, 1).reshape(B, -1, SKV)
    n_loads = 1 + len(HEAD_LOADS) + 2 + 1 + 2 * len(ORDER)
    n_messages = 2 * len(HEAD) + 26
    return pl.pallas_call(
        _body,
        out_shape=jax.ShapeDtypeStruct((B, SQ, DM), BF16),
        in_specs=[pl.BlockSpec(memory_space=pltpu.HBM)] * 5,
        out_specs=pl.BlockSpec(memory_space=pltpu.VMEM),
        scratch_shapes=[
            pltpu.VMEM((8, 2 * PAIR), F32),
            pltpu.VMEM((2, DM, PAIR), F32),
            pltpu.VMEM((2, PAIR, DM), F32),
            pltpu.VMEM((B, SQ, DM), F32),
            pltpu.VMEM((4, 2, B, PAIR, SKV), F32),
            pltpu.VMEM((4, 2, B, PAIR, SKV), F32),
            pltpu.VMEM((4, 2, 2, 256, 128), I32),
            pltpu.VMEM((4, 2, 2, 192, 128), I32),
            pltpu.VMEM((4, 8, 128), I32),
            pltpu.VMEM((B, SQ // 2, DM), I32),
            pltpu.VMEM((4, 2, B, SQ // 2, PAIR), I32),
            pltpu.VMEM((4, B * SQ, 128), F32),
            pltpu.SemaphoreType.DMA((n_loads,)),
            pltpu.SemaphoreType.DMA((n_messages,)),
            pltpu.SemaphoreType.DMA((n_messages,)),
            pltpu.SemaphoreType.REGULAR,
        ],
        compiler_params=pltpu.CompilerParams(
            collective_id=0, vmem_limit_bytes=48 << 20, disable_semaphore_checks=True),
    )(x, Wq, kt, vt, Wo)
```
